```python
import numpy as np

kernel_name = "dist_rope_attn_htp_bs_b2_sq512_d1024_hq8_dh128"

def setup_inputs():
    x = np.random.randn(8, 512, 1024).astype(np.float32)
    Wq = np.random.randn(1024, 4096).astype(np.float32) * 0.02
    Wk = np.random.randn(1024, 4096).astype(np.float32) * 0.02
    Wv = np.random.randn(1024, 4096).astype(np.float32) * 0.02
    Wo = np.random.randn(4096, 1024).astype(np.float32) * 0.02
    return {"x": x, "Wq": Wq, "Wk": Wk, "Wv": Wv, "Wo": Wo}

def reference(x, Wq, Wk, Wv, Wo):
    B, Sq, Hq, Dh = 8, 512, 32, 128
    inv = 1.0 / (10000.0 ** (np.arange(0, Dh, 2) / Dh))
    pos = np.arange(Sq)[:, None] * inv[None, :]
    cos = np.repeat(np.cos(pos), 2, axis=-1).astype(np.float32)
    sin = np.repeat(np.sin(pos), 2, axis=-1).astype(np.float32)
    def rot(t):
        t2 = t.reshape(B, Sq, Hq, Dh // 2, 2)
        t_r = np.stack([-t2[..., 1], t2[..., 0]], axis=-1).reshape(B, Sq, Hq, Dh)
        return t * cos[None, :, None, :] + t_r * sin[None, :, None, :]
    Q = rot((x @ Wq).reshape(B, Sq, Hq, Dh))
    K = rot((x @ Wk).reshape(B, Sq, Hq, Dh))
    V = (x @ Wv).reshape(B, Sq, Hq, Dh)
    s = np.einsum('bihd,bjhd->bhij', Q, K).astype(np.float32) * 0.08838834764831843
    s_max = s.max(axis=-1, keepdims=True)
    w = np.exp(s - s_max)
    w = w / w.sum(axis=-1, keepdims=True)
    ctx = np.einsum('bhij,bjhd->bihd', w, V).reshape(B, Sq, Hq * Dh)
    return ctx @ Wo
```

```python
import math

import jax
import jax.numpy as jnp
import numpy as np
from jax import lax
from jax.experimental import pallas as pl
from jax.experimental.pallas import tpu as pltpu

S, D, DH, NH = 512, 1024, 128, 8
NU = 8
SCALE = 0.08838834764831843 * math.log2(math.e)
BF = jnp.bfloat16
F32 = jnp.float32

_inv = 1.0 / (10000.0 ** (np.arange(0, DH, 2) / DH))
_pos = np.arange(S)[:, None] * _inv[None, :]
_COS = np.concatenate([np.cos(_pos), np.cos(_pos)], -1).astype(np.float32)
_SIN = np.concatenate([-np.sin(_pos), np.sin(_pos)], -1).astype(np.float32)


def _mm(a, b):
    return jnp.dot(a, b, preferred_element_type=F32)


def _mm_nt(a, b):
    return lax.dot_general(a, b, (((1,), (1,)), ((), ())), preferred_element_type=F32)


def _body(x_hbm, wq_hbm, wk_hbm, wv_hbm, wo_hbm, cos_ref, sin_ref, out_hbm,
          xst, wst, w, xbuf, ctx, psend, precv, own,
          ld_sem, xs_sem, xr_sem, ps_sem, pr_sem, out_sem):
    me = lax.axis_index("i")
    left = (me + 3) % 4
    right = (me + 1) % 4
    diag = (me + 2) % 4

    bar = pltpu.get_barrier_semaphore()
    for nbr in (left, right, diag):
        pl.semaphore_signal(bar, inc=1, device_id=(nbr,), device_id_type=pl.DeviceIdType.MESH)

    x_ld = [pltpu.make_async_copy(x_hbm.at[b], xst.at[b], ld_sem.at[b]) for b in range(2)]
    w_ld = [pltpu.make_async_copy(s, wst.at[i], ld_sem.at[2 + i])
            for i, s in enumerate((wq_hbm, wk_hbm, wv_hbm, wo_hbm))]
    x_ld[0].start()
    w_ld[0].start()
    w_ld[1].start()
    w_ld[2].start()
    x_ld[1].start()
    w_ld[3].start()

    def rcopy(src, dst, ssem, rsem, dev):
        return pltpu.make_async_remote_copy(
            src_ref=src, dst_ref=dst, send_sem=ssem, recv_sem=rsem,
            device_id=(dev,), device_id_type=pl.DeviceIdType.MESH)

    x_routes = [(0, 2, left), (0, 1, right), (0, 3, diag), (7, 6, left), (7, 5, right), (7, 4, diag)]
    x_sends = [rcopy(xbuf.at[s], xbuf.at[d], xs_sem.at[i], xr_sem.at[d - 1], dev)
               for i, (s, d, dev) in enumerate(x_routes)]

    x_ld[0].wait()
    xbuf[0] = xst[0].astype(BF)
    pl.semaphore_wait(bar, 3)
    for c in x_sends[:3]:
        c.start()

    src = lax.broadcasted_iota(jnp.int32, (DH, DH), 0)
    dst = lax.broadcasted_iota(jnp.int32, (DH, DH), 1)
    perm = (src == jnp.where(dst < 64, 2 * dst, 2 * dst - 127)).astype(BF)
    for i, sc in ((0, SCALE), (1, None)):
        w_ld[i].wait()
        for h in range(NH):
            t = wst[i, :, h * DH:(h + 1) * DH]
            if sc is not None:
                t = t * sc
            w[i, :, h * DH:(h + 1) * DH] = _mm(t.astype(BF), perm).astype(BF)
    w_ld[2].wait()
    w[2] = wst[2].astype(BF)
    x_ld[1].wait()
    xbuf[7] = xst[1].astype(BF)
    for c in x_sends[3:]:
        c.start()
    w_ld[3].wait()
    w[3] = wst[3].astype(BF)

    def p_recv(slot):
        return rcopy(psend.at[slot], precv.at[slot], ps_sem.at[slot], pr_sem.at[slot], me)

    def out_copy(b, r0, n):
        return pltpu.make_async_copy(own.at[b, pl.ds(r0, n)], out_hbm.at[b, pl.ds(r0, n)],
                                     out_sem.at[b * 4 + r0 // n])

    def finalize(b):
        for s in range(3):
            p_recv(3 * b + s).wait_recv()
        n = S // 4
        for c in range(4):
            rows = pl.ds(c * n, n)
            own[b, rows] = (own[b, rows] + precv[3 * b, rows].astype(F32)
                            + precv[3 * b + 1, rows].astype(F32) + precv[3 * b + 2, rows].astype(F32))
            out_copy(b, c * n, n).start()

    def unit(u, carry):
        remote = jnp.logical_and(u > 0, u < NU - 1)
        slot = jnp.clip(u - 1, 0, 5)

        @pl.when(remote)
        def _():
            rcopy(xbuf.at[u], xbuf.at[u], xs_sem.at[0], xr_sem.at[slot], me).wait_recv()

        xu = xbuf[u]
        cos = cos_ref[...]
        sin = sin_ref[...]
        for hp in range(NH // 2):
            cols = slice(hp * 2 * DH, (hp + 1) * 2 * DH)
            q2 = _mm(xu, w[0, :, cols])
            k2 = _mm(xu, w[1, :, cols])
            v2 = _mm(xu, w[2, :, cols]).astype(BF)
            for j in range(2):
                hs = slice(j * DH, (j + 1) * DH)
                q = q2[:, hs]
                k = k2[:, hs]
                q = (q * cos + pltpu.roll(q, 64, 1) * sin).astype(BF)
                k = (k * cos + pltpu.roll(k, 64, 1) * sin).astype(BF)
                s = _mm_nt(q, k)
                p = jnp.exp2(s - jnp.max(s, axis=-1, keepdims=True))
                l = jnp.sum(p, axis=-1, keepdims=True)
                o = _mm(p.astype(BF), v2[:, hs]) / l
                h = hp * 2 + j
                ctx[:, h * DH:(h + 1) * DH] = o.astype(BF)

        @pl.when(remote)
        def _():
            psend[slot] = _mm(ctx[...], w[3]).astype(BF)
            dev = jnp.where(jnp.logical_or(u == 1, u == 5), left,
                            jnp.where(jnp.logical_or(u == 2, u == 6), right, diag))
            rcopy(psend.at[slot], precv.at[slot], ps_sem.at[slot], pr_sem.at[slot], dev).start()

        @pl.when(jnp.logical_not(remote))
        def _():
            own[u // (NU - 1)] = _mm(ctx[...], w[3])

        @pl.when(u == 5)
        def _():
            finalize(0)

        return carry

    lax.fori_loop(0, NU, unit, 0)
    finalize(1)
    for c in x_sends:
        c.wait_send()
    for s in range(6):
        p_recv(s).wait_send()
    for b in range(2):
        for c in range(4):
            out_copy(b, c * (S // 4), S // 4).wait()


def pallas_dist_rope_attn_htp_bs_b2_sq512_d1024_hq8_dh128_kernel(x, Wq, Wk, Wv, Wo):
    any_spec = pl.BlockSpec(memory_space=pl.ANY)
    vmem_spec = pl.BlockSpec(memory_space=pltpu.VMEM)
    dma = pltpu.SemaphoreType.DMA
    return pl.pallas_call(
        _body,
        out_shape=jax.ShapeDtypeStruct((2, S, D), F32),
        in_specs=[any_spec] * 5 + [vmem_spec] * 2,
        out_specs=any_spec,
        scratch_shapes=[
            pltpu.VMEM((2, S, D), F32),
            pltpu.VMEM((4, D, D), F32),
            pltpu.VMEM((4, D, D), BF),
            pltpu.VMEM((NU, S, D), BF),
            pltpu.VMEM((S, D), BF),
            pltpu.VMEM((6, S, D), BF),
            pltpu.VMEM((6, S, D), BF),
            pltpu.VMEM((2, S, D), F32),
            dma((6,)), dma((6,)), dma((6,)), dma((6,)), dma((6,)), dma((8,)),
        ],
        compiler_params=pltpu.CompilerParams(collective_id=0, vmem_limit_bytes=100 * 1024 * 1024),
    )(x, Wq, Wk, Wv, Wo, jnp.asarray(_COS), jnp.asarray(_SIN))
```

```python
import math

import jax
import jax.numpy as jnp
from jax import lax
from jax.experimental import pallas as pl
from jax.experimental.pallas import tpu as pltpu

S, D, DH, NH = 512, 1024, 128, 8
NU = 8
SCALE = 0.08838834764831843 * math.log2(math.e)
BF = jnp.bfloat16
F32 = jnp.float32


def _mm(a, b):
    return jnp.dot(a, b, preferred_element_type=F32)


def _mm_nt(a, b):
    return lax.dot_general(a, b, (((1,), (1,)), ((), ())), preferred_element_type=F32)


def _body(x_hbm, wq_hbm, wk_hbm, wv_hbm, wo_hbm, out_hbm,
          xst, wst, w, xbuf, ctx, psend, precv, own, cos_ref, sin_ref,
          ld_sem, xs_sem, xr_sem, ps_sem, pr_sem, out_sem):
    me = lax.axis_index("i")
    left = (me + 3) % 4
    right = (me + 1) % 4
    diag = (me + 2) % 4

    bar = pltpu.get_barrier_semaphore()
    for nbr in (left, right, diag):
        pl.semaphore_signal(bar, inc=1, device_id=(nbr,), device_id_type=pl.DeviceIdType.MESH)

    NP = NH // 2
    x_ld = [pltpu.make_async_copy(x_hbm.at[b], xst.at[b], ld_sem.at[b]) for b in range(2)]
    wo_ld = pltpu.make_async_copy(wo_hbm, wst.at[3], ld_sem.at[2])
    w_ld = [[pltpu.make_async_copy(src.at[:, pl.ds(hp * 2 * DH, 2 * DH)],
                                   wst.at[i, :, pl.ds(hp * 2 * DH, 2 * DH)],
                                   ld_sem.at[3 + hp * 3 + i])
             for i, src in enumerate((wq_hbm, wk_hbm, wv_hbm))] for hp in range(NP)]
    x_ld[0].start()
    for hp in range(NP):
        for c in w_ld[hp]:
            c.start()
        if hp == 0:
            x_ld[1].start()
    wo_ld.start()

    lane = lax.broadcasted_iota(jnp.int32, (S, DH), 1)
    pos = lax.broadcasted_iota(jnp.int32, (S, DH), 0).astype(F32)
    ang = pos * jnp.exp((lane % 64).astype(F32) * (-math.log(10000.0) / 64))
    cos_ref[...] = jnp.cos(ang)
    sin_ref[...] = jnp.where(lane < 64, -1.0, 1.0) * jnp.sin(ang)

    def rcopy(src, dst, ssem, rsem, dev):
        return pltpu.make_async_remote_copy(
            src_ref=src, dst_ref=dst, send_sem=ssem, recv_sem=rsem,
            device_id=(dev,), device_id_type=pl.DeviceIdType.MESH)

    x_routes = [(0, 2, left), (0, 1, right), (0, 3, diag), (7, 6, left), (7, 5, right), (7, 4, diag)]
    x_sends = [rcopy(xbuf.at[s], xbuf.at[d], xs_sem.at[i], xr_sem.at[d - 1], dev)
               for i, (s, d, dev) in enumerate(x_routes)]

    x_ld[0].wait()
    xbuf[0] = xst[0].astype(BF)
    pl.semaphore_wait(bar, 3)
    for c in x_sends[:3]:
        c.start()

    src = lax.broadcasted_iota(jnp.int32, (DH, DH), 0)
    dst = lax.broadcasted_iota(jnp.int32, (DH, DH), 1)
    perm = (src == jnp.where(dst < 64, 2 * dst, 2 * dst - 127)).astype(BF)

    def prep_pair(hp):
        for i, sc in ((0, SCALE), (1, None)):
            w_ld[hp][i].wait()
            for h in (2 * hp, 2 * hp + 1):
                t = wst[i, :, h * DH:(h + 1) * DH]
                if sc is not None:
                    t = t * sc
                w[i, :, h * DH:(h + 1) * DH] = _mm(t.astype(BF), perm).astype(BF)
        w_ld[hp][2].wait()
        cols = slice(hp * 2 * DH, (hp + 1) * 2 * DH)
        w[2, :, cols] = wst[2, :, cols].astype(BF)
        if hp == 1:
            x_ld[1].wait()
            xbuf[7] = xst[1].astype(BF)
            for c in x_sends[3:]:
                c.start()

    def p_recv(slot):
        return rcopy(psend.at[slot], precv.at[slot], ps_sem.at[slot], pr_sem.at[slot], me)

    def out_copy(b, r0, n):
        return pltpu.make_async_copy(own.at[b, pl.ds(r0, n)], out_hbm.at[b, pl.ds(r0, n)],
                                     out_sem.at[b * 4 + r0 // n])

    def finalize(b, fresh):
        for s in range(3):
            p_recv(3 * b + s).wait_recv()
        n = S // 4
        for c in range(4):
            rows = pl.ds(c * n, n)
            mine = _mm(ctx[rows], w[3]) if fresh else own[b, rows]
            own[b, rows] = (mine + precv[3 * b, rows].astype(F32)
                            + precv[3 * b + 1, rows].astype(F32) + precv[3 * b + 2, rows].astype(F32))
            out_copy(b, c * n, n).start()

    def attention(u, first):
        xu = xbuf[u]
        cos = cos_ref[...]
        sin = sin_ref[...]
        for hp in range(NP):
            if first:
                prep_pair(hp)
            cols = slice(hp * 2 * DH, (hp + 1) * 2 * DH)
            q2 = _mm(xu, w[0, :, cols])
            k2 = _mm(xu, w[1, :, cols])
            v2 = _mm(xu, w[2, :, cols]).astype(BF)
            for j in range(2):
                hs = slice(j * DH, (j + 1) * DH)
                q = q2[:, hs]
                k = k2[:, hs]
                q = (q * cos + pltpu.roll(q, 64, 1) * sin).astype(BF)
                k = (k * cos + pltpu.roll(k, 64, 1) * sin).astype(BF)
                s = _mm_nt(q, k)
                p = jnp.exp2(s - jnp.max(s, axis=-1, keepdims=True))
                l = jnp.sum(p, axis=-1, keepdims=True)
                o = _mm(p.astype(BF), v2[:, hs]) / l
                h = hp * 2 + j
                ctx[:, h * DH:(h + 1) * DH] = o.astype(BF)

    attention(0, True)
    wo_ld.wait()
    w[3] = wst[3].astype(BF)
    own[0] = _mm(ctx[...], w[3])

    def unit(u, carry):
        slot = jnp.minimum(u - 1, 5)

        @pl.when(u < NU - 1)
        def _():
            rcopy(xbuf.at[u], xbuf.at[u], xs_sem.at[0], xr_sem.at[slot], me).wait_recv()

        attention(u, False)

        @pl.when(u < NU - 1)
        def _():
            psend[slot] = _mm(ctx[...], w[3]).astype(BF)
            dev = jnp.where(jnp.logical_or(u == 1, u == 5), left,
                            jnp.where(jnp.logical_or(u == 2, u == 6), right, diag))
            rcopy(psend.at[slot], precv.at[slot], ps_sem.at[slot], pr_sem.at[slot], dev).start()

        @pl.when(u == 5)
        def _():
            finalize(0, False)

        @pl.when(u == NU - 1)
        def _():
            finalize(1, True)

        return carry

    lax.fori_loop(1, NU, unit, 0)
    for c in x_sends:
        c.wait_send()
    for s in range(6):
        p_recv(s).wait_send()
    for b in range(2):
        for c in range(4):
            out_copy(b, c * (S // 4), S // 4).wait()


def pallas_dist_rope_attn_htp_bs_b2_sq512_d1024_hq8_dh128_kernel(x, Wq, Wk, Wv, Wo):
    any_spec = pl.BlockSpec(memory_space=pl.ANY)
    dma = pltpu.SemaphoreType.DMA
    return pl.pallas_call(
        _body,
        out_shape=jax.ShapeDtypeStruct((2, S, D), F32),
        in_specs=[any_spec] * 5,
        out_specs=any_spec,
        scratch_shapes=[
            pltpu.VMEM((2, S, D), F32),
            pltpu.VMEM((4, D, D), F32),
            pltpu.VMEM((4, D, D), BF),
            pltpu.VMEM((NU, S, D), BF),
            pltpu.VMEM((S, D), BF),
            pltpu.VMEM((6, S, D), BF),
            pltpu.VMEM((6, S, D), BF),
            pltpu.VMEM((2, S, D), F32),
            pltpu.VMEM((S, DH), F32),
            pltpu.VMEM((S, DH), F32),
            dma((15,)), dma((6,)), dma((6,)), dma((6,)), dma((6,)), dma((8,)),
        ],
        compiler_params=pltpu.CompilerParams(collective_id=0, vmem_limit_bytes=100 * 1024 * 1024),
    )(x, Wq, Wk, Wv, Wo)
```

```python
import math

import jax
import jax.numpy as jnp
from jax import lax
from jax.experimental import pallas as pl
from jax.experimental.pallas import tpu as pltpu

S, D, DH, NH = 512, 1024, 128, 8
NU = 8
SCALE = 0.08838834764831843 * math.log2(math.e)
BF = jnp.bfloat16
F32 = jnp.float32


def _mm(a, b):
    return jnp.dot(a, b, preferred_element_type=F32)


def _mm_nt(a, b):
    return lax.dot_general(a, b, (((1,), (1,)), ((), ())), preferred_element_type=F32)


def _body(x_hbm, wq_hbm, wk_hbm, wv_hbm, wo_hbm, own,
          xst, wst, w, xbuf, ctx, psend, precv, cos_ref, sin_ref,
          ld_sem, xs_sem, xr_sem, ps_sem, pr_sem):
    me = lax.axis_index("i")
    left = (me + 3) % 4
    right = (me + 1) % 4
    diag = (me + 2) % 4

    bar = pltpu.get_barrier_semaphore()
    for nbr in (left, right, diag):
        pl.semaphore_signal(bar, inc=1, device_id=(nbr,), device_id_type=pl.DeviceIdType.MESH)

    NP = NH // 2
    x_ld = [pltpu.make_async_copy(x_hbm.at[b], xst.at[b], ld_sem.at[b]) for b in range(2)]
    wo_ld = pltpu.make_async_copy(wo_hbm, wst.at[3], ld_sem.at[2])

    def w_ld(hp, i):
        cols = pl.ds(pl.multiple_of(hp * 2 * DH, 2 * DH), 2 * DH)
        return pltpu.make_async_copy((wq_hbm, wk_hbm, wv_hbm)[i].at[:, cols], wst.at[i, :, cols],
                                     ld_sem.at[3 + hp * 3 + i])

    x_ld[0].start()
    for hp in range(NP):
        for i in range(3):
            w_ld(hp, i).start()
        if hp == 0:
            x_ld[1].start()
    wo_ld.start()

    lane = lax.broadcasted_iota(jnp.int32, (S, DH), 1)
    pos = lax.broadcasted_iota(jnp.int32, (S, DH), 0).astype(F32)
    ang = pos * jnp.exp((lane % 64).astype(F32) * (-math.log(10000.0) / 64))
    cos_ref[...] = jnp.cos(ang)
    sin_ref[...] = jnp.where(lane < 64, -1.0, 1.0) * jnp.sin(ang)

    def rcopy(src, dst, ssem, rsem, dev):
        return pltpu.make_async_remote_copy(
            src_ref=src, dst_ref=dst, send_sem=ssem, recv_sem=rsem,
            device_id=(dev,), device_id_type=pl.DeviceIdType.MESH)

    x_routes = [(0, 2, left), (0, 1, right), (0, 3, diag), (7, 6, left), (7, 5, right), (7, 4, diag)]
    x_sends = [rcopy(xbuf.at[s], xbuf.at[d], xs_sem.at[i], xr_sem.at[d - 1], dev)
               for i, (s, d, dev) in enumerate(x_routes)]

    x_ld[0].wait()
    xbuf[0] = xst[0].astype(BF)
    pl.semaphore_wait(bar, 3)
    for c in x_sends[:3]:
        c.start()

    src = lax.broadcasted_iota(jnp.int32, (DH, DH), 0)
    dst = lax.broadcasted_iota(jnp.int32, (DH, DH), 1)
    perm = (src == jnp.where(dst < 64, 2 * dst, 2 * dst - 127)).astype(BF)

    def head(h):
        return pl.ds(pl.multiple_of(h * DH, DH), DH)

    def prep_pair(hp):
        for i, sc in ((0, SCALE), (1, None)):
            w_ld(hp, i).wait()
            for j in range(2):
                t = wst[i, :, head(2 * hp + j)]
                if sc is not None:
                    t = t * sc
                w[i, :, head(2 * hp + j)] = _mm(t.astype(BF), perm).astype(BF)
        w_ld(hp, 2).wait()
        for j in range(2):
            w[2, :, head(2 * hp + j)] = wst[2, :, head(2 * hp + j)].astype(BF)

    def p_recv(slot):
        return rcopy(psend.at[slot], precv.at[slot], ps_sem.at[slot], pr_sem.at[slot], me)

    def finalize(b, fresh):
        for s in range(3):
            p_recv(3 * b + s).wait_recv()
        n = S // 4
        for c in range(4):
            rows = pl.ds(c * n, n)
            mine = _mm(ctx[rows], w[3]) if fresh else own[b, rows]
            own[b, rows] = (mine + precv[3 * b, rows].astype(F32)
                            + precv[3 * b + 1, rows].astype(F32) + precv[3 * b + 2, rows].astype(F32))

    def pair(u, hp):
        @pl.when(u == 0)
        def _():
            prep_pair(hp)

        xu = xbuf[u]
        cos = cos_ref[...]
        sin = sin_ref[...]
        cols = pl.ds(pl.multiple_of(hp * 2 * DH, 2 * DH), 2 * DH)
        q2 = _mm(xu, w[0, :, cols])
        k2 = _mm(xu, w[1, :, cols])
        v2 = _mm(xu, w[2, :, cols]).astype(BF)
        for j in range(2):
            hs = slice(j * DH, (j + 1) * DH)
            q = q2[:, hs]
            k = k2[:, hs]
            q = (q * cos + pltpu.roll(q, 64, 1) * sin).astype(BF)
            k = (k * cos + pltpu.roll(k, 64, 1) * sin).astype(BF)
            s = _mm_nt(q, k)
            p = jnp.exp2(s - jnp.max(s, axis=-1, keepdims=True))
            l = jnp.sum(p, axis=-1, keepdims=True)
            o = _mm(p.astype(BF), v2[:, hs]) / l
            ctx[:, head(hp * 2 + j)] = o.astype(BF)

    def unit(u, carry):
        remote = jnp.logical_and(u > 0, u < NU - 1)
        slot = jnp.clip(u - 1, 0, 5)

        @pl.when(remote)
        def _():
            rcopy(xbuf.at[u], xbuf.at[u], xs_sem.at[0], xr_sem.at[slot], me).wait_recv()

        lax.fori_loop(0, NP, lambda hp, c: pair(u, hp), None)

        @pl.when(u == 0)
        def _():
            x_ld[1].wait()
            xbuf[7] = xst[1].astype(BF)
            for c in x_sends[3:]:
                c.start()
            wo_ld.wait()
            w[3] = wst[3].astype(BF)
            own[0] = _mm(ctx[...], w[3])

        @pl.when(remote)
        def _():
            psend[slot] = _mm(ctx[...], w[3]).astype(BF)
            dev = jnp.where(jnp.logical_or(u == 1, u == 5), left,
                            jnp.where(jnp.logical_or(u == 2, u == 6), right, diag))
            rcopy(psend.at[slot], precv.at[slot], ps_sem.at[slot], pr_sem.at[slot], dev).start()

        @pl.when(u == 5)
        def _():
            finalize(0, False)

        @pl.when(u == NU - 1)
        def _():
            finalize(1, True)

        return carry

    lax.fori_loop(0, NU, unit, 0)
    for c in x_sends:
        c.wait_send()
    for s in range(6):
        p_recv(s).wait_send()


def pallas_dist_rope_attn_htp_bs_b2_sq512_d1024_hq8_dh128_kernel(x, Wq, Wk, Wv, Wo):
    any_spec = pl.BlockSpec(memory_space=pltpu.MemorySpace.HBM)
    dma = pltpu.SemaphoreType.DMA
    return pl.pallas_call(
        _body,
        out_shape=jax.ShapeDtypeStruct((2, S, D), F32),
        in_specs=[any_spec] * 5,
        out_specs=pl.BlockSpec(memory_space=pltpu.VMEM),
        scratch_shapes=[
            pltpu.VMEM((2, S, D), F32),
            pltpu.VMEM((4, D, D), F32),
            pltpu.VMEM((4, D, D), BF),
            pltpu.VMEM((NU, S, D), BF),
            pltpu.VMEM((S, D), BF),
            pltpu.VMEM((6, S, D), BF),
            pltpu.VMEM((6, S, D), BF),
            pltpu.VMEM((S, DH), F32),
            pltpu.VMEM((S, DH), F32),
            dma((15,)), dma((6,)), dma((6,)), dma((6,)), dma((6,)),
        ],
        compiler_params=pltpu.CompilerParams(collective_id=0, vmem_limit_bytes=100 * 1024 * 1024),
    )(x, Wq, Wk, Wv, Wo)
```
